```python
import numpy as np

kernel_name = "dist_sparse_attn_blocksparse_qseq_b2_sq256_skv256_hq4_dh64"

def setup_inputs():
    x = np.random.randn(2, 1024, 512).astype(np.float32)
    Wq = np.random.randn(512, 1024).astype(np.float32) * 0.02
    K_ext = np.random.randn(2, 256, 16, 64).astype(np.float32)
    V_ext = np.random.randn(2, 256, 16, 64).astype(np.float32)
    Wo = np.random.randn(1024, 512).astype(np.float32) * 0.02
    return {"x": x, "Wq": Wq, "K_ext": K_ext, "V_ext": V_ext, "Wo": Wo}

def reference(x, Wq, K_ext, V_ext, Wo):
    B, Sq, Skv, Hq, Dh = 2, 1024, 256, 16, 64
    Q = (x @ Wq).reshape(B, Sq, Hq, Dh)
    qb = (np.arange(Sq) // 64)[:, None]
    kb = (np.arange(Skv) // 64)[None, :]
    mask = (qb == kb) | (kb == 0) | ((qb + kb) % 3 == 0)
    scores = np.einsum('bihd,bjhd->bhij', Q, K_ext).astype(np.float32) * 0.125
    scores = np.where(mask[None, None, :, :], scores, -1e9)
    scores_max = scores.max(axis=-1, keepdims=True)
    w = np.exp(scores - scores_max)
    row_keep = mask.any(axis=1)
    w_sum = np.where(row_keep[None, None, :, None], w.sum(axis=-1, keepdims=True), 1.0)
    w = w / w_sum
    w = np.where(row_keep[None, None, :, None], w, 0.0)
    ctx = np.einsum('bhij,bjhd->bihd', w, V_ext).reshape(B, Sq, Hq * Dh)
    return ctx @ Wo
```

```python
import contextlib
import functools

import jax
import jax.numpy as jnp
from jax import lax
from jax.experimental import pallas as pl
from jax.experimental.pallas import tpu as pltpu

f32, bf16 = jnp.float32, jnp.bfloat16
NT = (((1,), (1,)), ((), ()))
MESH = pl.DeviceIdType.MESH
QSCALE = 0.125 * 1.4426950408889634


def make_kernel(scopes=False, wq_pieces=(64, 128, 320), fwd_pieces=4, nosem=True, nobounds=False, out_dtype=f32):
    def scope(name):
        return jax.named_scope("s_" + name) if scopes else contextlib.nullcontext()

    def body(x_hbm, wq_hbm, k_hbm, v_hbm, wo_hbm, out_ref,
             x_f, x_b, wq_f, wo_f, k_f, v_f, kp, vp, wq_b, wo_b, ctx, acc,
             ld_wq, ld_x, ld_wo, ld_kv, snd_q, rcv_q, snd_o, rcv_o, ready):
        me = lax.axis_index("i")
        right = (me + 1) & 3
        left = (me + 3) & 3
        diag = (me + 2) & 3
        pair_of = [2 * me, 2 * me + 1, 2 * left, 2 * right + 1, 2 * left + 1, 2 * right, 2 * diag, 2 * diag + 1]
        if out_dtype == f32:
            acc = out_ref

        def remote(src, dst, ssem, rsem, dev):
            return pltpu.make_async_remote_copy(src, dst, ssem, rsem, device_id=(dev,), device_id_type=MESH)

        npc = len(wq_pieces)
        offs = [sum(wq_pieces[:i]) for i in range(npc)]
        wq_loads = [pltpu.make_async_copy(wq_hbm.at[pl.ds(o, n)], wq_f.at[pl.ds(o, n)], ld_wq.at[i])
                    for i, (o, n) in enumerate(zip(offs, wq_pieces))]
        x_load = pltpu.make_async_copy(x_hbm, x_f, ld_x)
        wo_load = pltpu.make_async_copy(wo_hbm, wo_f, ld_wo)
        kv_loads = [(pltpu.make_async_copy(k_hbm.at[:, pair_of[c]], k_f.at[c], ld_kv.at[c]),
                     pltpu.make_async_copy(v_hbm.at[:, pair_of[c]], v_f.at[c], ld_kv.at[c])) for c in range(8)]

        q_first = [[remote(wq_b.at[h, pl.ds(o, n)], wq_b.at[2 + h, pl.ds(o, n)], snd_q.at[h * npc + i], rcv_q.at[h * npc + i],
                           (right, left)[h]) for i, (o, n) in enumerate(zip(offs, wq_pieces))] for h in range(2)]
        q_second = [remote(wq_b.at[1 - h], wq_b.at[4 + h], snd_q.at[2 * npc + h], rcv_q.at[2 * npc + h], (right, left)[h]) for h in range(2)]
        q_fwd = [remote(wq_b.at[2 + h], wq_b.at[6 + h], snd_q.at[2 * npc + 2 + h], rcv_q.at[2 * npc + 2 + h], (right, left)[h]) for h in range(2)]
        o_first = [remote(wo_b.at[h], wo_b.at[2 + h], snd_o.at[h], rcv_o.at[h], (right, left)[h]) for h in range(2)]
        o_second = [remote(wo_b.at[1 - h], wo_b.at[4 + h], snd_o.at[2 + h], rcv_o.at[2 + h], (right, left)[h]) for h in range(2)]
        nb = 4 // fwd_pieces
        o_fwd = [[remote(wo_b.at[2 + h, pl.ds(n * nb, nb)], wo_b.at[6 + h, pl.ds(n * nb, nb)], snd_o.at[4 + h * fwd_pieces + n],
                         rcv_o.at[4 + h * fwd_pieces + n], (right, left)[h]) for n in range(fwd_pieces)] for h in range(2)]

        def kv_start(*cs):
            for c in cs:
                for d in kv_loads[c]:
                    d.start()

        with scope("start"):
            wq_loads[0].start()
            bar = pltpu.get_barrier_semaphore()

            @pl.when(me != 2)
            def _():
                for nbr in (left, right):
                    pl.semaphore_signal(bar, inc=1, device_id=(nbr,), device_id_type=MESH)
            for c in wq_loads[1:]:
                c.start()

        def cvt_wq(i):
            o, n = offs[i], wq_pieces[i]
            wq_loads[i].wait()
            w = wq_f[pl.ds(o, n), :] * QSCALE
            wq_b[0, pl.ds(o, n), :] = w[:, :128].astype(bf16)
            wq_b[1, pl.ds(o, n), :] = w[:, 128:].astype(bf16)

        with scope("wq0"):
            cvt_wq(0)
        with scope("barrier"):
            @pl.when(me != 0)
            def _():
                pl.semaphore_wait(bar, 2 - (me & 1))

        @pl.when(me == 2)
        def _():
            for nbr in (left, right):
                pl.semaphore_signal(ready, inc=1, device_id=(nbr,), device_id_type=MESH)

        early = [me >= 2, (me == 1) | (me == 2)]
        for i in range(npc):
            if i > 0:
                with scope(f"wq{i}"):
                    cvt_wq(i)
            for h in range(2):
                @pl.when(early[h])
                def _():
                    q_first[h][i].start()
        x_load.start()
        wo_load.start()
        for h in range(2):
            @pl.when(early[h])
            def _():
                q_second[h].start()

        with scope("late"):
            @pl.when(me == 0)
            def _():
                pl.semaphore_wait(bar, 2)

            @pl.when((me & 1) == 1)
            def _():
                pl.semaphore_wait(ready, 1)
            for h in range(2):
                @pl.when(jnp.logical_not(early[h]))
                def _():
                    for i in range(npc):
                        q_first[h][i].start()
                    q_second[h].start()

        with scope("wo"):
            wo_load.wait()
            kv_start(0, 1)
            for h in range(2):
                for n in range(4):
                    wo_b[h, n] = wo_f[h * 128:(h + 1) * 128, n * 128:(n + 1) * 128].astype(bf16)
            for h in range(2):
                o_first[h].start()

        ka = 3 - lax.rem(me, 3)
        b1 = jnp.where(ka == 2, 3, 2)
        b2 = jnp.where(ka == 1, 3, 1)

        def vis(j, kb):
            qb = 4 * me + j
            return ((qb == kb) | (lax.rem(qb + kb, 3) == 0)).astype(jnp.int32)

        vis1 = (vis(1, b1), vis(2, b1))
        vis2 = (vis(1, b2), vis(2, b2))

        def perm(t):
            t1, t2 = t[:, :128], t[:, 128:]
            x = jnp.where(ka == 2, pltpu.roll(t2, 64, 1), t2)
            keep = (lax.broadcasted_iota(jnp.int32, (128, 128), 1) < 64) | (ka == 1)
            return jnp.where(keep, t1, x), jnp.where(keep, x, t1)

        def prep(c):
            for b in range(2):
                k1, k2 = perm(k_f[c, b])
                v1, v2 = perm(v_f[c, b])
                kp[c, b, 0:128, :] = k1.astype(bf16).T
                kp[c, b, 128:256, :] = k2.astype(bf16).T
                vp[c, b, :, 0:128] = v1.astype(bf16)
                vp[c, b, :, 128:256] = v2.astype(bf16)

        def sm(s):
            m = jnp.max(s, axis=0, keepdims=True)
            p = jnp.exp2(s - m)
            l = jnp.sum(p, axis=0, keepdims=True)
            return p, pl.reciprocal(l, approx=True)

        def attend(c):
            lane64 = lax.broadcasted_iota(jnp.int32, (64, 128), 1) < 64
            m1 = jnp.where(lane64, vis1[0], vis1[1]) > 0
            m2 = jnp.where(lane64, vis2[0], vis2[1]) > 0
            q = jnp.dot(x_b[...], wq_b[c], preferred_element_type=f32)
            lane = lax.broadcasted_iota(jnp.int32, (256, 128), 1) < 64
            S, P, O = {}, {}, {}
            for b in range(2):
                qb = q[b * 256:(b + 1) * 256]
                kk = kp[c, b]
                la = kk[:128]
                lb = jnp.concatenate([kk[:64], kk[128:]], 0)
                for h in range(2):
                    qh = jnp.where(lane, qb, 0.0) if h == 0 else jnp.where(lane, 0.0, qb)
                    qa = jnp.concatenate([qh[0:64], qh[192:256]], 0).astype(bf16)
                    qbb = qh[64:192].astype(bf16)
                    S[b, h, 0] = lax.dot_general(la, qa, NT, preferred_element_type=f32)
                    S[b, h, 1] = lax.dot_general(lb, qbb, NT, preferred_element_type=f32)
            for b in range(2):
                for h in range(2):
                    P[b, h, 0] = sm(S[b, h, 0])
                    s = S[b, h, 1]
                    s = jnp.concatenate([s[:64], jnp.where(m1, s[64:128], -1e9), jnp.where(m2, s[128:], -1e9)], 0)
                    P[b, h, 1] = sm(s)
            for b in range(2):
                for h in range(2):
                    v = vp[c, b, h * 64:(h + 1) * 64, :]
                    pa, ra = P[b, h, 0]
                    O[b, h, 0] = jnp.dot(v[:, :128], pa.astype(bf16), preferred_element_type=f32) * ra
                    pb, rb = P[b, h, 1]
                    pfull = jnp.concatenate([pb[:64], jnp.zeros((64, 128), f32), pb[64:]], 0).astype(bf16)
                    O[b, h, 1] = jnp.dot(v, pfull, preferred_element_type=f32) * rb
            for b in range(2):
                ca = jnp.concatenate([O[b, 0, 0], O[b, 1, 0]], 0).astype(bf16).T
                cb = jnp.concatenate([O[b, 0, 1], O[b, 1, 1]], 0).astype(bf16).T
                ctx[c, pl.ds(b * 256, 64), :] = ca[:64]
                ctx[c, pl.ds(b * 256 + 64, 128), :] = cb
                ctx[c, pl.ds(b * 256 + 192, 64), :] = ca[64:]

        def kv_wait(c):
            for d in kv_loads[c]:
                d.wait()

        def proj(cs, n):
            rhs = jnp.concatenate([wo_b[c, n] for c in cs], 0)
            parts = 1 if len(cs) >= 4 else 4 // len(cs)
            rows = 512 // parts
            res = []
            for r in range(parts):
                lhs = jnp.concatenate([ctx[c, pl.ds(r * rows, rows), :] for c in cs], 1)
                res.append(jnp.dot(lhs, rhs, preferred_element_type=f32))
            return jnp.concatenate(res, 0)

        with scope("x"):
            x_load.wait()
            x_b[...] = x_f[...].astype(bf16)

        for p in range(4):
            if p == 3:
                with scope("wait_o1"):
                    for h in range(2):
                        o_first[h].wait_recv()
                    for n in range(fwd_pieces):
                        for h in range(2):
                            o_fwd[h][n].start()
                with scope("proj1"):
                    for n in range(4):
                        acc[:, n * 128:(n + 1) * 128] = proj((0, 1, 2, 3), n)
            with scope(f"prep{p}"):
                kv_wait(2 * p)
                kv_wait(2 * p + 1)
                if p < 3:
                    kv_start(2 * p + 2, 2 * p + 3)
                prep(2 * p)
                prep(2 * p + 1)
            with scope(f"wait{p}"):
                if p == 1:
                    for h in range(2):
                        for d in q_first[h]:
                            d.wait_recv()
                    for h in range(2):
                        q_fwd[h].start()
                    for h in range(2):
                        o_second[h].start()
                elif p == 2:
                    for h in range(2):
                        q_second[h].wait_recv()
                elif p == 3:
                    for h in range(2):
                        q_fwd[h].wait_recv()
            with scope(f"attn{p}"):
                attend(2 * p)
                attend(2 * p + 1)

        with scope("wait_o2"):
            for h in range(2):
                o_second[h].wait_recv()
        with scope("proj2"):
            for n in range(4):
                acc[:, n * 128:(n + 1) * 128] += proj((4, 5), n)
        with scope("sendwait"):
            for h in range(2):
                for d in q_first[h]:
                    d.wait_send()
                q_second[h].wait_send()
                q_fwd[h].wait_send()
                o_first[h].wait_send()
                o_second[h].wait_send()
        for m in range(fwd_pieces):
            if m == fwd_pieces - 1:
                with scope("sendwait2"):
                    for h in range(2):
                        for d in o_fwd[h]:
                            d.wait_send()
            with scope(f"wait_o3_{m}"):
                for h in range(2):
                    o_fwd[h][m].wait_recv()
            with scope(f"proj3_{m}"):
                for n in range(m * nb, (m + 1) * nb):
                    out_ref[:, n * 128:(n + 1) * 128] = (acc[:, n * 128:(n + 1) * 128] + proj((6, 7), n)).astype(out_dtype)

    def kernel(x, Wq, K_ext, V_ext, Wo):
        kt = jnp.transpose(K_ext, (0, 2, 3, 1)).reshape(2, 8, 128, 256)
        vt = jnp.transpose(V_ext, (0, 2, 3, 1)).reshape(2, 8, 128, 256)
        hbm = pl.BlockSpec(memory_space=pltpu.HBM)
        npc = len(wq_pieces)
        out = pl.pallas_call(
            body,
            out_shape=jax.ShapeDtypeStruct((512, 512), out_dtype),
            in_specs=[hbm] * 5,
            out_specs=pl.BlockSpec(memory_space=pltpu.VMEM),
            scratch_shapes=[
                pltpu.VMEM((512, 512), f32), pltpu.VMEM((512, 512), bf16),
                pltpu.VMEM((512, 256), f32), pltpu.VMEM((256, 512), f32),
                pltpu.VMEM((8, 2, 128, 256), f32), pltpu.VMEM((8, 2, 128, 256), f32),
                pltpu.VMEM((8, 2, 256, 128), bf16), pltpu.VMEM((8, 2, 128, 256), bf16),
                pltpu.VMEM((8, 512, 128), bf16), pltpu.VMEM((8, 4, 128, 128), bf16), pltpu.VMEM((8, 512, 128), bf16),
                pltpu.VMEM((512, 512), f32),
                pltpu.SemaphoreType.DMA((npc,)), pltpu.SemaphoreType.DMA, pltpu.SemaphoreType.DMA, pltpu.SemaphoreType.DMA((8,)),
                pltpu.SemaphoreType.DMA((2 * npc + 4,)), pltpu.SemaphoreType.DMA((2 * npc + 4,)),
                pltpu.SemaphoreType.DMA((4 + 2 * fwd_pieces,)), pltpu.SemaphoreType.DMA((4 + 2 * fwd_pieces,)),
                pltpu.SemaphoreType.REGULAR,
            ],
            compiler_params=pltpu.CompilerParams(collective_id=0, vmem_limit_bytes=64 * 2**20,
                                                 disable_semaphore_checks=nosem, disable_bounds_checks=nobounds),
        )(x.reshape(512, 512), Wq, kt, vt, Wo)
        return out.reshape(2, 256, 512)

    return kernel


_kernel = make_kernel()


def pallas_dist_sparse_attn_blocksparse_qseq_b2_sq256_skv256_hq4_dh64_kernel(x, Wq, K_ext, V_ext, Wo):
    return _kernel(x, Wq, K_ext, V_ext, Wo)
```

```python
import jax
import jax.numpy as jnp
from jax import lax
from jax.experimental import pallas as pl
from jax.experimental.pallas import tpu as pltpu

f32, bf16, i32 = jnp.float32, jnp.bfloat16, jnp.int32
MESH = pl.DeviceIdType.MESH
SCALE = 0.125 * 1.4426950408889634
NUM_REMOTE = 44

SIGN = 0x80008000 - (1 << 32)
HIGH = 0x78007800
LOW = 0x87FF87FF - (1 << 32)
EXP_ONE = 0x00800080
RAW = 255


def _tree(f, xs):
    while len(xs) > 1:
        xs = [f(*xs[i:i + 2]) if i + 1 < len(xs) else xs[i] for i in range(0, len(xs), 2)]
    return xs[0]


def _words(w):
    return [w[8 * i:8 * i + 8] for i in range(w.shape[0] // 8)]


def _describe(words):
    top = _tree(jnp.maximum, [pltpu.bitcast(x & 0x7F800000, f32) for w in words for x in (w, w << 16)])
    top = jnp.max(jnp.max(top, axis=0, keepdims=True), axis=1, keepdims=True)
    base = jnp.maximum((pltpu.bitcast(top, i32) >> 23) - 15, 0)
    floor = jnp.maximum(base - 16, 0)
    words = [w | SIGN for w in words]
    below = ~_tree(jnp.bitwise_or,
                   [lax.shift_right_logical((w - base * EXP_ONE) & SIGN, i) for i, w in enumerate(words)])
    reachable = _tree(jnp.bitwise_and, [w - floor * EXP_ONE for w in words]) & SIGN
    ok = ((below & (below - 1)) == 0) & (reachable == SIGN)
    ok = jnp.min(jnp.min(jnp.where(ok, 1.0, 0.0), axis=0, keepdims=True), axis=1, keepdims=True) > 0.5
    return jnp.where(ok, base, RAW), lax.clz(below)


def _pack(words, raw):
    high = jnp.where(raw, 0, HIGH)
    out = []
    for q in range(0, len(words), 4):
        first = words[q]
        third = ((first << 3) & 0x38003800) | (lax.shift_right_logical(first, 1) & 0x40004000)
        for w, bits in zip(words[q + 1:q + 4], (first << 11, first << 7, third)):
            out.append((w & ~high) | (bits & high))
    return jnp.concatenate(out, 0)


def _unpack(packed, first, code, odd, quad):
    raw = code == RAW
    keep = jnp.where(raw, -1, LOW)
    turn = jnp.where(raw, 0, (-code & 15) * EXP_ONE)
    base = jnp.where(raw, 0, code * EXP_ONE)
    which = jnp.where(raw | (odd == 32), 16, odd & 15)
    lower = base - jnp.where(odd < 16, 0x08000000, 0x0800)
    a, b, c = packed
    low = ((a & HIGH) >> 11) | ((b & HIGH) >> 7) | ((c & 0x38003800) >> 3) | ((c << 1) & SIGN)
    words = [jnp.where(raw, first, low), a & keep, b & keep, c & keep]
    return [((w + turn) & keep) + jnp.where(which == 4 * quad + i, lower, base) for i, w in enumerate(words)]


def _body(x_hbm, wq_hbm, k_hbm, v_hbm, wo_hbm, out_ref,
          x_f, x_b, wq_f, wo_f, k_f, v_f, k_b, v_b, w_own, lead, pk, firsts, redo, side, q_b, o_t, ctx, acc,
          ld_wq, ld_x, ld_wo, ld_kv, snd, rcv, ready):
    me = lax.axis_index("i")
    right, diag, left = (me + 1) & 3, (me + 2) & 3, (me + 3) & 3
    owner = (0, 0, 1, 2, 1, 2, 3, 3)
    half_of = (0, 1, 0, 1, 1, 0, 0, 1)
    pair_of = [2 * (me, left, right, diag)[owner[c]] + half_of[c] for c in range(8)]

    sems = iter(range(NUM_REMOTE))

    def remote(src, dst, h):
        i = next(sems)
        return pltpu.make_async_remote_copy(src, dst, snd.at[i], rcv.at[i],
                                            device_id=((right, left)[h],), device_id_type=MESH)

    def each_way(f):
        return [f(h) for h in range(2)]

    q_first = each_way(lambda h: [
        remote(lead.at[h, pl.ds(0, 24)], pk.at[0, 2 + h, pl.ds(0, 24)], h),
        remote(lead.at[h, pl.ds(24, 72)], pk.at[0, 2 + h, pl.ds(24, 72)], h),
        remote(pk.at[0, h, pl.ds(96, 96)], pk.at[0, 2 + h, pl.ds(96, 96)], h)])
    o_first = each_way(lambda h: remote(pk.at[1, h], pk.at[1, 2 + h], h))
    second = [each_way(lambda h: remote(pk.at[m, 1 - h], pk.at[m, 4 + h], h)) for m in range(2)]
    q_fwd = each_way(lambda h: remote(pk.at[0, 2 + h], pk.at[0, 6 + h], h))
    o_fwd = each_way(lambda h: [remote(pk.at[1, 2 + h, pl.ds(o, n)], pk.at[1, 6 + h, pl.ds(o, n)], h)
                                for o, n in ((0, 48), (48, 48), (96, 48), (144, 24), (168, 24))])
    side_own = [each_way(lambda h: remote(side.at[m, 0], side.at[m, 1 + h], h)) for m in range(2)]
    side_fwd = [remote(side.at[m, 1 + m], side.at[m, 3], m) for m in range(2)]
    q_redo = each_way(lambda h: remote(pk.at[0, h, pl.ds(0, 96)], redo.at[h], h))
    raw_first = [each_way(lambda h: remote(firsts.at[m, h], firsts.at[m, 2 + h], h)) for m in range(2)]
    raw_second = [each_way(lambda h: remote(firsts.at[m, 1 - h], firsts.at[m, 4 + h], h)) for m in range(2)]
    raw_fwd = [each_way(lambda h: remote(firsts.at[m, 2 + h], firsts.at[m, 6 + h], h)) for m in range(2)]

    h0 = jnp.where(me == 1, 1, 0)
    halves = (h0, 1 - h0)
    wq_rows = ((0, 64), (64, 192), (256, 256))
    wq_loads = [[pltpu.make_async_copy(wq_hbm.at[pl.ds(o, n), pl.ds(pl.multiple_of(128 * halves[s], 128), 128)],
                                       wq_f.at[s, pl.ds(o, n)], ld_wq.at[3 * s + i])
                 for i, (o, n) in enumerate(wq_rows)] for s in range(2)]
    x_loads = [pltpu.make_async_copy(x_hbm.at[pl.ds(256 * b, 256)], x_f.at[pl.ds(256 * b, 256)], ld_x.at[b])
               for b in range(2)]
    wo_load = pltpu.make_async_copy(wo_hbm, wo_f, ld_wo)
    kv_loads = [(pltpu.make_async_copy(k_hbm.at[:, pair_of[c]], k_f.at[c], ld_kv.at[c]),
                 pltpu.make_async_copy(v_hbm.at[:, pair_of[c]], v_f.at[c], ld_kv.at[c])) for c in range(8)]

    def kv_start(c):
        for d in kv_loads[c]:
            d.start()

    def kv_wait(c):
        for d in kv_loads[c]:
            d.wait()

    codes = {}

    def own_words(m, half, o, n):
        return _words(pltpu.bitcast(w_own[m, half, pl.ds(o, n), :], i32))

    def encode(m, half, g):
        words = own_words(m, half, 256 * g, 256)
        code, odd = _describe(words)
        pk[m, half, pl.ds(96 * g, 96), :] = _pack(words, code == RAW)
        firsts[m, half, pl.ds(32 * g, 32), :] = jnp.concatenate(words[::4], 0)
        return code << (16 * half + 8 * g), odd << (16 * half + 8 * g)

    def write_side(m, groups):
        code = _tree(jnp.bitwise_or, [c for c, _ in groups])
        odd = _tree(jnp.bitwise_or, [o for _, o in groups])
        row = lax.broadcasted_iota(i32, (8, 128), 0) & 3
        side[m, 0] = odd | ((lax.shift_right_logical(jnp.broadcast_to(code, (8, 128)), 2 * row) & 0x03030303) << 6)
        codes[m, 0] = code[0, 0]

    def read_side(m, o):
        rows = [(lax.shift_right_logical(side[m, o, r:r + 1, :], 6) & 0x03030303) << (2 * r) for r in range(4)]
        codes[m, o] = _tree(jnp.bitwise_or, rows)[0, 0]

    def code_of(m, c, g):
        return lax.shift_right_logical(codes[m, owner[c]], 16 * half_of[c] + 8 * g) & 255

    def odd_of(m, c, g):
        return lax.shift_right_logical(side[m, owner[c]], 16 * half_of[c] + 8 * g) & 63

    def has_raw(m, *cs):
        return _tree(jnp.bitwise_or, [code_of(m, c, g) == RAW for c in cs for g in range(2)])

    def weights(m, c, u):
        if c < 2:
            return w_own[m, c, pl.ds(64 * u, 64), :]
        words = _unpack(_words(pk[m, c, pl.ds(24 * u, 24), :]), firsts[m, c, pl.ds(8 * u, 8), :],
                        code_of(m, c, u // 4), odd_of(m, c, u // 4), u % 4)
        return pltpu.bitcast(jnp.concatenate(words, 0), bf16)

    ka = 3 - lax.rem(me, 3)
    b1 = jnp.where(ka == 2, 3, 2)
    b2 = jnp.where(ka == 1, 3, 1)

    def sees(j, kb):
        qb = 4 * me + j
        return ((qb == kb) | (lax.rem(qb + kb, 3) == 0)).astype(i32)

    def prep(c):
        keep = (lax.broadcasted_iota(i32, (128, 128), 1) < 64) | (ka == 1)
        for b in range(2):
            k_b[c, b] = k_f[c, b].astype(bf16).T
            lo, hi = v_f[c, b, :, 0:128], v_f[c, b, :, 128:256]
            hi = jnp.where(ka == 2, pltpu.roll(hi, 64, 1), hi)
            v_b[c, b, 0] = jnp.where(keep, lo, hi).astype(bf16)
            v_b[c, b, 1] = jnp.where(keep, hi, lo).astype(bf16)

    def project_q(c):
        w = jnp.concatenate([weights(0, c, u) for u in range(8)], 0)
        q = jnp.dot(x_b[...], w, preferred_element_type=f32)
        first = lax.broadcasted_iota(i32, (512, 128), 1) < 64
        q_b[c, 0] = jnp.where(first, q, 0.0).astype(bf16)
        q_b[c, 1] = jnp.where(first, 0.0, q).astype(bf16)

    def scores(c):
        s = {}
        for b in range(2):
            k0 = k_b[c, b, 0:64, :]
            ks = [k_b[c, b, pl.ds(pl.multiple_of(64 * kb, 64), 64), :] for kb in (ka, b1, b2)]
            keys = (jnp.concatenate([k0, ks[0]], 0), jnp.concatenate([k0, ks[1], ks[2]], 0))
            for h in range(2):
                q = (jnp.concatenate([q_b[c, h, pl.ds(256 * b, 64), :], q_b[c, h, pl.ds(256 * b + 192, 64), :]], 0),
                     q_b[c, h, pl.ds(256 * b + 64, 128), :])
                for t in range(2):
                    s[b, h, t] = lax.dot_general(keys[t], q[t], (((1,), (1,)), ((), ())),
                                                 preferred_element_type=f32)
        return s

    def attend(c, s):
        first = lax.broadcasted_iota(i32, (64, 128), 1) < 64
        seen = [jnp.where(first, sees(1, kb), sees(2, kb)) > 0 for kb in (b1, b2)]
        p = {}
        for (b, h, t), x in s.items():
            if t == 1:
                x = jnp.concatenate(
                    [x[:64], jnp.where(seen[0], x[64:128], -1e9), jnp.where(seen[1], x[128:], -1e9)], 0)
            e = jnp.exp2(x - jnp.max(x, axis=0, keepdims=True))
            p[b, h, t] = e, 1.0 / jnp.sum(e, axis=0, keepdims=True)
        for (b, h, t), (e, inv) in p.items():
            v = v_b[c, b, 0, 64 * h:64 * h + 64, :]
            if t == 1:
                v = jnp.concatenate([v, v_b[c, b, 1, 64 * h:64 * h + 64, :]], 1)
                e = jnp.concatenate([e[:64], jnp.zeros((64, 128), f32), e[64:]], 0)
            o = jnp.dot(v, e.astype(bf16), preferred_element_type=f32) * inv
            tile, place = (c, h) if c < 6 else (6 + h, c - 6)
            o_t[tile, b, t, pl.ds(64 * place, 64), :] = o.astype(bf16)

    def put_ctx(c):
        for b in range(2):
            a = o_t[c, b, 0].T
            ctx[c, pl.ds(256 * b, 64), :] = a[:64]
            ctx[c, pl.ds(256 * b + 64, 128), :] = o_t[c, b, 1].T
            ctx[c, pl.ds(256 * b + 192, 64), :] = a[64:]

    def project_out(cs, w, parts):
        rows = 512 // parts
        return jnp.concatenate(
            [jnp.dot(jnp.concatenate([ctx[c, pl.ds(r * rows, rows), :] for c in cs], 1), w,
                     preferred_element_type=f32) for r in range(parts)], 0)

    def wo_tiles(cs, n):
        return jnp.concatenate([weights(1, c, u) for c in cs for u in (2 * n, 2 * n + 1)], 0)

    wq_loads[0][0].start()
    barrier = pltpu.get_barrier_semaphore()

    @pl.when(me != 2)
    def _():
        for other in (left, right):
            pl.semaphore_signal(barrier, inc=1, device_id=(other,), device_id_type=MESH)

    wq_loads[1][0].start()
    for i in (1, 2):
        for s in range(2):
            wq_loads[s][i].start()

    @pl.when(me != 0)
    def _():
        pl.semaphore_wait(barrier, 2 - (me & 1))

    @pl.when(me == 2)
    def _():
        for other in (left, right):
            pl.semaphore_signal(ready, inc=1, device_id=(other,), device_id_type=MESH)

    may_send = (me >= 2, (me == 1) | (me == 2))
    groups = []
    for i, (o, n) in enumerate(wq_rows):
        for s in range(2):
            wq_loads[s][i].wait()
            w_own[0, halves[s], pl.ds(o, n), :] = wq_f[s, pl.ds(o, n), :].astype(bf16)
            if i < 2:
                lead[halves[s], pl.ds(3 * o // 8, 3 * n // 8), :] = _pack(own_words(0, halves[s], o, n), False)
            else:
                groups.append(encode(0, halves[s], 1))
            for h in range(2):
                pl.when(may_send[h] & (halves[s] == h))(q_first[h][i].start)
        if i == 0:
            for d in x_loads:
                d.start()
    kv_start(0)

    @pl.when((me & 1) == 1)
    def _():
        pl.semaphore_wait(ready, 1)
        for h in range(2):
            @pl.when(jnp.logical_not(may_send[h]))
            def _():
                for d in q_first[h]:
                    d.start()

    write_side(0, groups + [encode(0, half, 0) for half in range(2)])

    @pl.when(me == 0)
    def _():
        pl.semaphore_wait(barrier, 2)
        for pieces in zip(*q_first):
            for d in pieces:
                d.start()

    for h in range(2):
        side_own[0][h].start()
        second[0][h].start()

    @pl.when(has_raw(0, 0, 1))
    def _():
        for h in range(2):
            pl.when(code_of(0, h, 0) == RAW)(q_redo[h].start)
            pl.when(has_raw(0, h))(raw_first[0][h].start)
            pl.when(has_raw(0, 1 - h))(raw_second[0][h].start)

    for b in range(2):
        x_loads[b].wait()
        x_b[pl.ds(256 * b, 256), :] = (x_f[pl.ds(256 * b, 256), :] * SCALE).astype(bf16)
        if b == 0:
            wo_load.start()
    project_q(0)

    kv_wait(0)
    kv_start(1)
    prep(0)
    project_q(1)

    wo_load.wait()
    kv_start(2)
    for h in range(2):
        for n in range(4):
            w_own[1, h, pl.ds(128 * n, 128), :] = wo_f[128 * h:128 * h + 128, 128 * n:128 * n + 128].astype(bf16)
    write_side(1, [encode(1, h, g) for h in range(2) for g in range(2)])
    for h in range(2):
        side_own[1][h].start()
        o_first[h].start()

    @pl.when(has_raw(1, 0, 1))
    def _():
        for h in range(2):
            pl.when(has_raw(1, h))(raw_first[1][h].start)
            pl.when(has_raw(1, 1 - h))(raw_second[1][h].start)

    kv_start(3)
    attend(0, scores(0))

    kv_wait(1)
    kv_start(4)
    for h in range(2):
        side_own[0][h].wait_recv()
    for h in range(2):
        read_side(0, 1 + h)
    side_fwd[0].start()
    for h in range(2):
        for d in q_first[h]:
            d.wait_recv()

    @pl.when(has_raw(0, 2, 3))
    def _():
        for h in range(2):
            @pl.when(code_of(0, 2 + h, 0) == RAW)
            def _():
                q_redo[h].wait_recv()
                pk[0, 2 + h, 0:96, :] = redo[h]

            pl.when(has_raw(0, 2 + h))(raw_first[0][h].wait_recv)
            pl.when(has_raw(0, 2 + h))(raw_fwd[0][h].start)

    for h in range(2):
        q_fwd[h].start()
        second[1][h].start()
    put_ctx(0)
    prep(1)
    project_q(2)

    kv_wait(2)
    kv_start(5)
    prep(2)
    s = scores(1)
    project_q(3)
    attend(1, s)

    kv_wait(3)
    kv_start(6)
    put_ctx(1)
    prep(3)
    attend(2, scores(2))

    kv_wait(4)
    kv_start(7)
    for h in range(2):
        second[0][h].wait_recv()

    @pl.when(has_raw(0, 4, 5))
    def _():
        for h in range(2):
            pl.when(has_raw(0, 4 + h))(raw_second[0][h].wait_recv)

    for c in (3, 4):
        if c == 4:
            kv_wait(5)
        put_ctx(c - 1)
        prep(c + 1)
        s = scores(c)
        project_q(c + 1)
        attend(c, s)

    kv_wait(6)
    kv_wait(7)
    for h in range(2):
        side_own[1][h].wait_recv()
    side_fwd[0].wait_recv()
    for h in range(2):
        read_side(1, 1 + h)
    read_side(0, 3)
    side_fwd[1].start()
    for h in range(2):
        o_first[h].wait_recv()

    @pl.when(has_raw(1, 2, 3, 4, 5))
    def _():
        for h in range(2):
            pl.when(has_raw(1, 2 + h))(raw_first[1][h].wait_recv)
            pl.when(has_raw(1, 2 + h))(raw_fwd[1][h].start)
            pl.when(has_raw(1, 4 + h))(raw_second[1][h].wait_recv)

    for pieces in zip(*o_fwd):
        for d in pieces:
            d.start()
    put_ctx(4)
    prep(6)
    prep(7)
    s = scores(5)
    for n in range(4):
        acc[:, 128 * n:128 * n + 128] = project_out((0, 1, 2, 3), wo_tiles((0, 1, 2, 3), n), 1)
        if n == 1:
            attend(5, s)

    for h in range(2):
        q_fwd[h].wait_recv()

    @pl.when(has_raw(0, 6, 7))
    def _():
        for h in range(2):
            pl.when(has_raw(0, 6 + h))(raw_fwd[0][h].wait_recv)

    put_ctx(5)
    project_q(6)
    s = scores(6)
    project_q(7)
    attend(6, s)
    attend(7, scores(7))

    for h in range(2):
        second[1][h].wait_recv()
    side_fwd[1].wait_recv()
    read_side(1, 3)
    put_ctx(6)
    put_ctx(7)
    for n in range(4):
        acc[:, 128 * n:128 * n + 128] += project_out((4, 5), wo_tiles((4, 5), n), 2)

    @pl.when(has_raw(1, 6, 7))
    def _():
        for h in range(2):
            pl.when(has_raw(1, 6 + h))(raw_fwd[1][h].wait_recv)

    for i, (n, hs) in enumerate(((0, (0, 1)), (1, (0, 1)), (2, (0, 1)), (3, (0,)), (3, (1,)))):
        if i == 2:
            for h in range(2):
                for d in (*q_first[h], o_first[h], second[0][h], second[1][h], q_fwd[h], *o_fwd[h],
                          side_own[0][h], side_own[1][h], side_fwd[h]):
                    d.wait_send()

            @pl.when(has_raw(0, 0, 1, 2, 3) | has_raw(1, 0, 1, 2, 3))
            def _():
                for h in range(2):
                    pl.when(code_of(0, h, 0) == RAW)(q_redo[h].wait_send)
                    for m in range(2):
                        pl.when(has_raw(m, h))(raw_first[m][h].wait_send)
                        pl.when(has_raw(m, 1 - h))(raw_second[m][h].wait_send)
                        pl.when(has_raw(m, 2 + h))(raw_fwd[m][h].wait_send)

        for h in range(2):
            o_fwd[h][i].wait_recv()
        cols = pl.ds(128 * n, 128)
        w = jnp.concatenate([weights(1, c, 2 * n + h) for h in hs for c in (6, 7)], 0)
        total = acc[:, cols] + project_out([6 + h for h in hs], w, 4 // len(hs))
        if hs[-1] == 1:
            out_ref[:, cols] = total.astype(out_ref.dtype)
        else:
            acc[:, cols] = total


def pallas_dist_sparse_attn_blocksparse_qseq_b2_sq256_skv256_hq4_dh64_kernel(
    x: jax.Array,
    Wq: jax.Array,
    K_ext: jax.Array,
    V_ext: jax.Array,
    Wo: jax.Array,
):
    kt = jnp.transpose(K_ext, (0, 2, 3, 1)).reshape(2, 8, 128, 256)
    vt = jnp.transpose(V_ext, (0, 2, 3, 1)).reshape(2, 8, 128, 256)
    vmem, dma = pltpu.VMEM, pltpu.SemaphoreType.DMA
    out = pl.pallas_call(
        _body,
        out_shape=jax.ShapeDtypeStruct((512, 512), bf16),
        in_specs=[pl.BlockSpec(memory_space=pltpu.HBM)] * 5,
        out_specs=pl.BlockSpec(memory_space=pltpu.VMEM),
        scratch_shapes=[
            vmem((512, 512), f32), vmem((512, 512), bf16),
            vmem((2, 512, 128), f32), vmem((256, 512), f32),
            vmem((8, 2, 128, 256), f32), vmem((8, 2, 128, 256), f32),
            vmem((8, 2, 256, 128), bf16), vmem((8, 2, 2, 128, 128), bf16),
            vmem((2, 2, 512, 128), bf16), vmem((2, 96, 128), i32),
            vmem((2, 8, 192, 128), i32), vmem((2, 8, 64, 128), i32),
            vmem((2, 96, 128), i32), vmem((2, 4, 8, 128), i32),
            vmem((8, 2, 512, 128), bf16), vmem((8, 2, 2, 128, 128), bf16),
            vmem((8, 512, 128), bf16), vmem((512, 512), f32),
            dma((6,)), dma((2,)), dma, dma((8,)),
            dma((NUM_REMOTE,)), dma((NUM_REMOTE,)), pltpu.SemaphoreType.REGULAR,
        ],
        compiler_params=pltpu.CompilerParams(
            collective_id=0, vmem_limit_bytes=64 * 2**20, disable_semaphore_checks=True),
    )(x.reshape(512, 512), Wq, kt, vt, Wo)
    return out.reshape(2, 256, 512)
```

```python
import jax
import jax.numpy as jnp
from jax import lax
from jax.experimental import pallas as pl
from jax.experimental.pallas import tpu as pltpu

f32, bf16, i32 = jnp.float32, jnp.bfloat16, jnp.int32
MESH = pl.DeviceIdType.MESH
SCALE = 0.125 * 1.4426950408889634
NUM_REMOTE = 46

SIGN = 0x80008000 - (1 << 32)
HIGH = 0x78007800
LOW = 0x87FF87FF - (1 << 32)
EXP_ONE = 0x00800080
RAW = 255


def _tree(f, xs):
    while len(xs) > 1:
        xs = [f(*xs[i:i + 2]) if i + 1 < len(xs) else xs[i] for i in range(0, len(xs), 2)]
    return xs[0]


def _words(w):
    return [w[8 * i:8 * i + 8] for i in range(w.shape[0] // 8)]


def _describe(words):
    top = _tree(jnp.maximum, [pltpu.bitcast(x & 0x7F800000, f32) for w in words for x in (w, w << 16)])
    top = jnp.max(jnp.max(top, axis=0, keepdims=True), axis=1, keepdims=True)
    base = jnp.maximum((pltpu.bitcast(top, i32) >> 23) - 15, 0)
    floor = jnp.maximum(base - 16, 0)
    words = [w | SIGN for w in words]
    below = ~_tree(jnp.bitwise_or,
                   [lax.shift_right_logical((w - base * EXP_ONE) & SIGN, i) for i, w in enumerate(words)])
    reachable = _tree(jnp.bitwise_and, [w - floor * EXP_ONE for w in words]) & SIGN
    ok = ((below & (below - 1)) == 0) & (reachable == SIGN)
    ok = jnp.min(jnp.min(jnp.where(ok, 1.0, 0.0), axis=0, keepdims=True), axis=1, keepdims=True) > 0.5
    return jnp.where(ok, base, RAW), lax.clz(below)


def _pack(words, raw):
    high = jnp.where(raw, 0, HIGH)
    out = []
    for q in range(0, len(words), 4):
        first = words[q]
        third = ((first << 3) & 0x38003800) | (lax.shift_right_logical(first, 1) & 0x40004000)
        for w, bits in zip(words[q + 1:q + 4], (first << 11, first << 7, third)):
            out.append((w & ~high) | (bits & high))
    return jnp.concatenate(out, 0)


def _unpack(packed, first, code, odd, quad):
    raw = code == RAW
    keep = jnp.where(raw, -1, LOW)
    turn = jnp.where(raw, 0, (-code & 15) * EXP_ONE)
    base = jnp.where(raw, 0, code * EXP_ONE)
    which = jnp.where(raw | (odd == 32), 16, odd & 15)
    lower = base - jnp.where(odd < 16, 0x08000000, 0x0800)
    a, b, c = packed
    low = ((a & HIGH) >> 11) | ((b & HIGH) >> 7) | ((c & 0x38003800) >> 3) | ((c << 1) & SIGN)
    words = [jnp.where(raw, first, low), a & keep, b & keep, c & keep]
    return [((w + turn) & keep) + jnp.where(which == 4 * quad + i, lower, base) for i, w in enumerate(words)]


def _body(x_hbm, wq_hbm, k_hbm, v_hbm, wo_hbm, out_ref,
          x_f, x_b, wq_f, wo_f, k_f, v_f, k_b, v_b, w_own, lead, pk, firsts, redo, side, q_b, o_t, ctx, acc,
          ld_wq, ld_x, ld_wo, ld_kv, snd, rcv, ready):
    me = lax.axis_index("i")
    right, diag, left = (me + 1) & 3, (me + 2) & 3, (me + 3) & 3
    owner = (0, 0, 1, 2, 1, 2, 3, 3)
    half_of = (0, 1, 0, 1, 1, 0, 0, 1)
    pair_of = [2 * (me, left, right, diag)[owner[c]] + half_of[c] for c in range(8)]

    sems = iter(range(NUM_REMOTE))

    def remote(src, dst, h):
        i = next(sems)
        return pltpu.make_async_remote_copy(src, dst, snd.at[i], rcv.at[i],
                                            device_id=((right, left)[h],), device_id_type=MESH)

    def each_way(f):
        return [f(h) for h in range(2)]

    q_first = each_way(lambda h: [
        *(remote(lead.at[h, pl.ds(o, n)], pk.at[0, 2 + h, pl.ds(o, n)], h) for o, n in ((0, 24), (24, 24), (48, 48))),
        remote(pk.at[0, h, pl.ds(96, 96)], pk.at[0, 2 + h, pl.ds(96, 96)], h)])
    o_first = each_way(lambda h: remote(pk.at[1, h], pk.at[1, 2 + h], h))
    second = [each_way(lambda h: remote(pk.at[m, 1 - h], pk.at[m, 4 + h], h)) for m in range(2)]
    q_fwd = each_way(lambda h: remote(pk.at[0, 2 + h], pk.at[0, 6 + h], h))
    o_fwd = each_way(lambda h: [remote(pk.at[1, 2 + h, pl.ds(o, n)], pk.at[1, 6 + h, pl.ds(o, n)], h)
                                for o, n in ((0, 48), (48, 48), (96, 48), (144, 24), (168, 24))])
    side_own = [each_way(lambda h: remote(side.at[m, 0], side.at[m, 1 + h], h)) for m in range(2)]
    side_fwd = [remote(side.at[m, 1 + m], side.at[m, 3], m) for m in range(2)]
    q_redo = each_way(lambda h: remote(pk.at[0, h, pl.ds(0, 96)], redo.at[h], h))
    raw_first = [each_way(lambda h: remote(firsts.at[m, h], firsts.at[m, 2 + h], h)) for m in range(2)]
    raw_second = [each_way(lambda h: remote(firsts.at[m, 1 - h], firsts.at[m, 4 + h], h)) for m in range(2)]
    raw_fwd = [each_way(lambda h: remote(firsts.at[m, 2 + h], firsts.at[m, 6 + h], h)) for m in range(2)]

    h0 = jnp.where(me == 1, 1, 0)
    halves = (h0, 1 - h0)
    wq_rows = ((0, 64), (64, 64), (128, 128), (256, 256))
    wq_loads = [[pltpu.make_async_copy(wq_hbm.at[pl.ds(o, n), pl.ds(pl.multiple_of(128 * halves[s], 128), 128)],
                                       wq_f.at[s, pl.ds(o, n)], ld_wq.at[4 * s + i])
                 for i, (o, n) in enumerate(wq_rows)] for s in range(2)]
    x_loads = [pltpu.make_async_copy(x_hbm.at[pl.ds(256 * b, 256)], x_f.at[pl.ds(256 * b, 256)], ld_x.at[b])
               for b in range(2)]
    wo_load = pltpu.make_async_copy(wo_hbm, wo_f, ld_wo)
    kv_loads = [(pltpu.make_async_copy(k_hbm.at[:, pair_of[c]], k_f.at[c], ld_kv.at[c]),
                 pltpu.make_async_copy(v_hbm.at[:, pair_of[c]], v_f.at[c], ld_kv.at[c])) for c in range(8)]

    def kv_start(c):
        for d in kv_loads[c]:
            d.start()

    def kv_wait(c):
        for d in kv_loads[c]:
            d.wait()

    codes = {}

    def own_words(m, half, o, n):
        return _words(pltpu.bitcast(w_own[m, half, pl.ds(o, n), :], i32))

    def encode(m, half, g):
        words = own_words(m, half, 256 * g, 256)
        code, odd = _describe(words)
        pk[m, half, pl.ds(96 * g, 96), :] = _pack(words, code == RAW)
        firsts[m, half, pl.ds(32 * g, 32), :] = jnp.concatenate(words[::4], 0)
        return code << (16 * half + 8 * g), odd << (16 * half + 8 * g)

    def write_side(m, groups):
        code = _tree(jnp.bitwise_or, [c for c, _ in groups])
        odd = _tree(jnp.bitwise_or, [o for _, o in groups])
        row = lax.broadcasted_iota(i32, (8, 128), 0) & 3
        side[m, 0] = odd | ((lax.shift_right_logical(jnp.broadcast_to(code, (8, 128)), 2 * row) & 0x03030303) << 6)
        codes[m, 0] = code[0, 0]

    def read_side(m, o):
        rows = [(lax.shift_right_logical(side[m, o, r:r + 1, :], 6) & 0x03030303) << (2 * r) for r in range(4)]
        codes[m, o] = _tree(jnp.bitwise_or, rows)[0, 0]

    def code_of(m, c, g):
        return lax.shift_right_logical(codes[m, owner[c]], 16 * half_of[c] + 8 * g) & 255

    def odd_of(m, c, g):
        return lax.shift_right_logical(side[m, owner[c]], 16 * half_of[c] + 8 * g) & 63

    def has_raw(m, *cs):
        return _tree(jnp.bitwise_or, [code_of(m, c, g) == RAW for c in cs for g in range(2)])

    def weights(m, c, u):
        if c < 2:
            return w_own[m, c, pl.ds(64 * u, 64), :]
        words = _unpack(_words(pk[m, c, pl.ds(24 * u, 24), :]), firsts[m, c, pl.ds(8 * u, 8), :],
                        code_of(m, c, u // 4), odd_of(m, c, u // 4), u % 4)
        return pltpu.bitcast(jnp.concatenate(words, 0), bf16)

    ka = 3 - lax.rem(me, 3)
    b1 = jnp.where(ka == 2, 3, 2)
    b2 = jnp.where(ka == 1, 3, 1)

    def sees(j, kb):
        qb = 4 * me + j
        return ((qb == kb) | (lax.rem(qb + kb, 3) == 0)).astype(i32)

    def prep(c):
        keep = (lax.broadcasted_iota(i32, (128, 128), 1) < 64) | (ka == 1)
        for b in range(2):
            k_b[c, b] = k_f[c, b].astype(bf16).T
            lo, hi = v_f[c, b, :, 0:128], v_f[c, b, :, 128:256]
            hi = jnp.where(ka == 2, pltpu.roll(hi, 64, 1), hi)
            v_b[c, b, 0] = jnp.where(keep, lo, hi).astype(bf16)
            v_b[c, b, 1] = jnp.where(keep, hi, lo).astype(bf16)

    def project_q(c):
        w = jnp.concatenate([weights(0, c, u) for u in range(8)], 0)
        q = jnp.dot(x_b[...], w, preferred_element_type=f32)
        first = lax.broadcasted_iota(i32, (512, 128), 1) < 64
        q_b[c, 0] = jnp.where(first, q, 0.0).astype(bf16)
        q_b[c, 1] = jnp.where(first, 0.0, q).astype(bf16)

    def scores(c):
        s = {}
        for b in range(2):
            k0 = k_b[c, b, 0:64, :]
            ks = [k_b[c, b, pl.ds(pl.multiple_of(64 * kb, 64), 64), :] for kb in (ka, b1, b2)]
            keys = (jnp.concatenate([k0, ks[0]], 0), jnp.concatenate([k0, ks[1], ks[2]], 0))
            for h in range(2):
                q = (jnp.concatenate([q_b[c, h, pl.ds(256 * b, 64), :], q_b[c, h, pl.ds(256 * b + 192, 64), :]], 0),
                     q_b[c, h, pl.ds(256 * b + 64, 128), :])
                for t in range(2):
                    s[b, h, t] = lax.dot_general(keys[t], q[t], (((1,), (1,)), ((), ())),
                                                 preferred_element_type=f32)
        return s

    def attend(c, s):
        first = lax.broadcasted_iota(i32, (64, 128), 1) < 64
        seen = [jnp.where(first, sees(1, kb), sees(2, kb)) > 0 for kb in (b1, b2)]
        p = {}
        for (b, h, t), x in s.items():
            if t == 1:
                x = jnp.concatenate(
                    [x[:64], jnp.where(seen[0], x[64:128], -1e9), jnp.where(seen[1], x[128:], -1e9)], 0)
            e = jnp.exp2(x - jnp.max(x, axis=0, keepdims=True))
            p[b, h, t] = e, 1.0 / jnp.sum(e, axis=0, keepdims=True)
        for (b, h, t), (e, inv) in p.items():
            v = v_b[c, b, 0, 64 * h:64 * h + 64, :]
            if t == 1:
                v = jnp.concatenate([v, v_b[c, b, 1, 64 * h:64 * h + 64, :]], 1)
                e = jnp.concatenate([e[:64], jnp.zeros((64, 128), f32), e[64:]], 0)
            o = jnp.dot(v, e.astype(bf16), preferred_element_type=f32) * inv
            tile, place = (c, h) if c < 6 else (6 + h, c - 6)
            o_t[tile, b, t, pl.ds(64 * place, 64), :] = o.astype(bf16)

    def put_ctx(c):
        for b in range(2):
            a = o_t[c, b, 0].T
            ctx[c, pl.ds(256 * b, 64), :] = a[:64]
            ctx[c, pl.ds(256 * b + 64, 128), :] = o_t[c, b, 1].T
            ctx[c, pl.ds(256 * b + 192, 64), :] = a[64:]

    def project_out(cs, w, parts):
        rows = 512 // parts
        return jnp.concatenate(
            [jnp.dot(jnp.concatenate([ctx[c, pl.ds(r * rows, rows), :] for c in cs], 1), w,
                     preferred_element_type=f32) for r in range(parts)], 0)

    def wo_tiles(cs, n):
        return jnp.concatenate([weights(1, c, u) for c in cs for u in (2 * n, 2 * n + 1)], 0)

    wq_order = ((0, 0), (0, 1), (1, 0), (1, 1), (0, 2), (1, 2), (0, 3), (1, 3))
    for s, i in wq_order[:2]:
        wq_loads[s][i].start()
    barrier = pltpu.get_barrier_semaphore()

    @pl.when(me != 2)
    def _():
        for other in (left, right):
            pl.semaphore_signal(barrier, inc=1, device_id=(other,), device_id_type=MESH)

    for s, i in wq_order[2:]:
        wq_loads[s][i].start()

    @pl.when(me != 0)
    def _():
        pl.semaphore_wait(barrier, 2 - (me & 1))

    @pl.when(me == 2)
    def _():
        for other in (left, right):
            pl.semaphore_signal(ready, inc=1, device_id=(other,), device_id_type=MESH)

    may_send = (me >= 2, (me == 1) | (me == 2))
    groups = []
    for s, i in wq_order:
        o, n = wq_rows[i]
        wq_loads[s][i].wait()
        w_own[0, halves[s], pl.ds(o, n), :] = wq_f[s, pl.ds(o, n), :].astype(bf16)
        if i < 3:
            lead[halves[s], pl.ds(3 * o // 8, 3 * n // 8), :] = _pack(own_words(0, halves[s], o, n), False)
        else:
            groups.append(encode(0, halves[s], 1))
        for h in range(2):
            pl.when(may_send[h] & (halves[s] == h))(q_first[h][i].start)
        if (s, i) == wq_order[1]:
            for d in x_loads:
                d.start()
    kv_start(0)

    @pl.when((me & 1) == 1)
    def _():
        pl.semaphore_wait(ready, 1)
        for h in range(2):
            @pl.when(jnp.logical_not(may_send[h]))
            def _():
                for d in q_first[h]:
                    d.start()

    write_side(0, groups + [encode(0, half, 0) for half in range(2)])

    @pl.when(me == 0)
    def _():
        pl.semaphore_wait(barrier, 2)
        for pieces in zip(*q_first):
            for d in pieces:
                d.start()

    for h in range(2):
        side_own[0][h].start()
        second[0][h].start()

    @pl.when(has_raw(0, 0, 1))
    def _():
        for h in range(2):
            pl.when(code_of(0, h, 0) == RAW)(q_redo[h].start)
            pl.when(has_raw(0, h))(raw_first[0][h].start)
            pl.when(has_raw(0, 1 - h))(raw_second[0][h].start)

    for b in range(2):
        x_loads[b].wait()
        x_b[pl.ds(256 * b, 256), :] = (x_f[pl.ds(256 * b, 256), :] * SCALE).astype(bf16)
        if b == 0:
            wo_load.start()
    project_q(0)

    kv_wait(0)
    kv_start(1)
    prep(0)
    project_q(1)

    wo_load.wait()
    kv_start(2)
    for h in range(2):
        for n in range(4):
            w_own[1, h, pl.ds(128 * n, 128), :] = wo_f[128 * h:128 * h + 128, 128 * n:128 * n + 128].astype(bf16)
    write_side(1, [encode(1, h, g) for h in range(2) for g in range(2)])
    for h in range(2):
        side_own[1][h].start()
        o_first[h].start()

    @pl.when(has_raw(1, 0, 1))
    def _():
        for h in range(2):
            pl.when(has_raw(1, h))(raw_first[1][h].start)
            pl.when(has_raw(1, 1 - h))(raw_second[1][h].start)

    kv_start(3)
    attend(0, scores(0))

    kv_wait(1)
    kv_start(4)
    for h in range(2):
        side_own[0][h].wait_recv()
    for h in range(2):
        read_side(0, 1 + h)
    side_fwd[0].start()
    for h in range(2):
        for d in q_first[h]:
            d.wait_recv()

    @pl.when(has_raw(0, 2, 3))
    def _():
        for h in range(2):
            @pl.when(code_of(0, 2 + h, 0) == RAW)
            def _():
                q_redo[h].wait_recv()
                pk[0, 2 + h, 0:96, :] = redo[h]

            pl.when(has_raw(0, 2 + h))(raw_first[0][h].wait_recv)
            pl.when(has_raw(0, 2 + h))(raw_fwd[0][h].start)

    for h in range(2):
        q_fwd[h].start()
        second[1][h].start()
    put_ctx(0)
    prep(1)
    project_q(2)

    kv_wait(2)
    kv_start(5)
    prep(2)
    s = scores(1)
    project_q(3)
    attend(1, s)

    kv_wait(3)
    kv_start(6)
    put_ctx(1)
    prep(3)
    attend(2, scores(2))

    kv_wait(4)
    kv_start(7)
    for h in range(2):
        second[0][h].wait_recv()

    @pl.when(has_raw(0, 4, 5))
    def _():
        for h in range(2):
            pl.when(has_raw(0, 4 + h))(raw_second[0][h].wait_recv)

    for c in (3, 4):
        if c == 4:
            kv_wait(5)
        put_ctx(c - 1)
        prep(c + 1)
        s = scores(c)
        project_q(c + 1)
        attend(c, s)

    kv_wait(6)
    kv_wait(7)
    for h in range(2):
        side_own[1][h].wait_recv()
    side_fwd[0].wait_recv()
    for h in range(2):
        read_side(1, 1 + h)
    read_side(0, 3)
    side_fwd[1].start()
    for h in range(2):
        o_first[h].wait_recv()

    @pl.when(has_raw(1, 2, 3, 4, 5))
    def _():
        for h in range(2):
            pl.when(has_raw(1, 2 + h))(raw_first[1][h].wait_recv)
            pl.when(has_raw(1, 2 + h))(raw_fwd[1][h].start)
            pl.when(has_raw(1, 4 + h))(raw_second[1][h].wait_recv)

    for pieces in zip(*o_fwd):
        for d in pieces:
            d.start()
    put_ctx(4)
    prep(6)
    prep(7)
    s = scores(5)
    for n in range(4):
        acc[:, 128 * n:128 * n + 128] = project_out((0, 1, 2, 3), wo_tiles((0, 1, 2, 3), n), 1)
        if n == 1:
            attend(5, s)

    for h in range(2):
        q_fwd[h].wait_recv()

    @pl.when(has_raw(0, 6, 7))
    def _():
        for h in range(2):
            pl.when(has_raw(0, 6 + h))(raw_fwd[0][h].wait_recv)

    put_ctx(5)
    project_q(6)
    s = scores(6)
    project_q(7)
    attend(6, s)
    attend(7, scores(7))

    for h in range(2):
        second[1][h].wait_recv()
    side_fwd[1].wait_recv()
    read_side(1, 3)
    put_ctx(6)
    put_ctx(7)
    for n in range(4):
        acc[:, 128 * n:128 * n + 128] += project_out((4, 5), wo_tiles((4, 5), n), 2)

    @pl.when(has_raw(1, 6, 7))
    def _():
        for h in range(2):
            pl.when(has_raw(1, 6 + h))(raw_fwd[1][h].wait_recv)

    for i, (n, hs) in enumerate(((0, (0, 1)), (1, (0, 1)), (2, (0, 1)), (3, (0,)), (3, (1,)))):
        if i == 2:
            for h in range(2):
                for d in (*q_first[h], o_first[h], second[0][h], second[1][h], q_fwd[h], *o_fwd[h],
                          side_own[0][h], side_own[1][h], side_fwd[h]):
                    d.wait_send()

            @pl.when(has_raw(0, 0, 1, 2, 3) | has_raw(1, 0, 1, 2, 3))
            def _():
                for h in range(2):
                    pl.when(code_of(0, h, 0) == RAW)(q_redo[h].wait_send)
                    for m in range(2):
                        pl.when(has_raw(m, h))(raw_first[m][h].wait_send)
                        pl.when(has_raw(m, 1 - h))(raw_second[m][h].wait_send)
                        pl.when(has_raw(m, 2 + h))(raw_fwd[m][h].wait_send)

        for h in range(2):
            o_fwd[h][i].wait_recv()
        cols = pl.ds(128 * n, 128)
        w = jnp.concatenate([weights(1, c, 2 * n + h) for h in hs for c in (6, 7)], 0)
        total = acc[:, cols] + project_out([6 + h for h in hs], w, 4 // len(hs))
        if hs[-1] == 1:
            out_ref[:, cols] = total.astype(out_ref.dtype)
        else:
            acc[:, cols] = total


def pallas_dist_sparse_attn_blocksparse_qseq_b2_sq256_skv256_hq4_dh64_kernel(
    x: jax.Array,
    Wq: jax.Array,
    K_ext: jax.Array,
    V_ext: jax.Array,
    Wo: jax.Array,
):
    kt = jnp.transpose(K_ext, (0, 2, 3, 1)).reshape(2, 8, 128, 256)
    vt = jnp.transpose(V_ext, (0, 2, 3, 1)).reshape(2, 8, 128, 256)
    vmem, dma = pltpu.VMEM, pltpu.SemaphoreType.DMA
    out = pl.pallas_call(
        _body,
        out_shape=jax.ShapeDtypeStruct((512, 512), bf16),
        in_specs=[pl.BlockSpec(memory_space=pltpu.HBM)] * 5,
        out_specs=pl.BlockSpec(memory_space=pltpu.VMEM),
        scratch_shapes=[
            vmem((512, 512), f32), vmem((512, 512), bf16),
            vmem((2, 512, 128), f32), vmem((256, 512), f32),
            vmem((8, 2, 128, 256), f32), vmem((8, 2, 128, 256), f32),
            vmem((8, 2, 256, 128), bf16), vmem((8, 2, 2, 128, 128), bf16),
            vmem((2, 2, 512, 128), bf16), vmem((2, 96, 128), i32),
            vmem((2, 8, 192, 128), i32), vmem((2, 8, 64, 128), i32),
            vmem((2, 96, 128), i32), vmem((2, 4, 8, 128), i32),
            vmem((8, 2, 512, 128), bf16), vmem((8, 2, 2, 128, 128), bf16),
            vmem((8, 512, 128), bf16), vmem((512, 512), f32),
            dma((8,)), dma((2,)), dma, dma((8,)),
            dma((NUM_REMOTE,)), dma((NUM_REMOTE,)), pltpu.SemaphoreType.REGULAR,
        ],
        compiler_params=pltpu.CompilerParams(
            collective_id=0, vmem_limit_bytes=64 * 2**20, disable_semaphore_checks=True),
    )(x.reshape(512, 512), Wq, kt, vt, Wo)
    return out.reshape(2, 256, 512)
```

```python
import jax
import jax.numpy as jnp
from jax import lax
from jax.experimental import pallas as pl
from jax.experimental.pallas import tpu as pltpu

f32, bf16, i32 = jnp.float32, jnp.bfloat16, jnp.int32
MESH = pl.DeviceIdType.MESH
SCALE = 0.125 * 1.4426950408889634
NUM_REMOTE = 44

SIGN = 0x80008000 - (1 << 32)
HIGH = 0x78007800
LOW = 0x87FF87FF - (1 << 32)
EXP_ONE = 0x00800080
FULL = 255


def _tree(f, xs):
    while len(xs) > 1:
        xs = [f(*xs[i:i + 2]) if i + 1 < len(xs) else xs[i] for i in range(0, len(xs), 2)]
    return xs[0]


def _words(w):
    return [w[8 * i:8 * i + 8] for i in range(w.shape[0] // 8)]


def _describe(words):
    top = _tree(jnp.maximum, [pltpu.bitcast(x & 0x7F800000, f32) for w in words for x in (w, w << 16)])
    top = jnp.max(jnp.max(top, axis=0, keepdims=True), axis=1, keepdims=True)
    base = jnp.maximum((pltpu.bitcast(top, i32) >> 23) - 15, 0)
    floor = jnp.maximum(base - 16, 0)
    words = [w | SIGN for w in words]
    below = ~_tree(jnp.bitwise_or,
                   [lax.shift_right_logical((w - base * EXP_ONE) & SIGN, i) for i, w in enumerate(words)])
    reachable = _tree(jnp.bitwise_and, [w - floor * EXP_ONE for w in words]) & SIGN
    ok = ((below & (below - 1)) == 0) & (reachable == SIGN)
    ok = jnp.min(jnp.min(jnp.where(ok, 1.0, 0.0), axis=0, keepdims=True), axis=1, keepdims=True) > 0.5
    return jnp.where(ok, base, FULL), lax.clz(below)


def _pack(words):
    out = []
    for q in range(0, len(words), 4):
        first = words[q]
        third = ((first << 3) & 0x38003800) | (lax.shift_right_logical(first, 1) & 0x40004000)
        for w, bits in zip(words[q + 1:q + 4], ((first << 11) & HIGH, (first << 7) & HIGH, third)):
            out.append((w & LOW) | bits)
    return jnp.concatenate(out, 0)


def _pack_high(words):
    h = [w & HIGH for w in words]
    return jnp.concatenate([(h[q] >> 11) | (h[q + 1] >> 7) | (h[q + 2] >> 3) | (h[q + 3] << 1)
                            for q in range(0, len(words), 4)], 0)


def _unpack(packed, high, code, odd, quad):
    full = code == FULL
    a, b, c = packed
    lows = [((a & HIGH) >> 11) | ((b & HIGH) >> 7) | ((c & 0x38003800) >> 3) | ((c << 1) & SIGN),
            a & LOW, b & LOW, c & LOW]
    sent = (high << 11, high << 7, high << 3, lax.shift_right_logical(high, 1))
    turn = jnp.where(full, 0, (-code & 15) * EXP_ONE)
    base = code * EXP_ONE
    lower = base - jnp.where(odd < 16, 0x08000000, 0x0800)
    which = jnp.where(odd == 32, 16, odd & 15)
    return [((w + turn) & LOW) + jnp.where(full, h & HIGH, jnp.where(which == 4 * quad + i, lower, base))
            for i, (w, h) in enumerate(zip(lows, sent))]


def _body(x_hbm, wq_hbm, k_hbm, v_hbm, wo_hbm, out_ref,
          x_f, x_b, wq_f, wo_f, k_f, v_f, k_b, v_b, w_own, pk, high, side, q_b, o_t, ctx, acc,
          ld_wq, ld_x, ld_wo, ld_kv, snd, rcv, ready):
    me = lax.axis_index("i")
    right, diag, left = (me + 1) & 3, (me + 2) & 3, (me + 3) & 3
    owner = (0, 0, 1, 2, 1, 2, 3, 3)
    half_of = (0, 1, 0, 1, 1, 0, 0, 1)
    pair_of = [2 * (me, left, right, diag)[owner[c]] + half_of[c] for c in range(8)]

    sems = iter(range(NUM_REMOTE))

    def remote(src, dst, h):
        i = next(sems)
        return pltpu.make_async_remote_copy(src, dst, snd.at[i], rcv.at[i],
                                            device_id=((right, left)[h],), device_id_type=MESH)

    def each_way(f):
        return [f(h) for h in range(2)]

    q_first = each_way(lambda h: [remote(pk.at[0, h, pl.ds(o, n)], pk.at[0, 2 + h, pl.ds(o, n)], h)
                                  for o, n in ((0, 24), (24, 24), (48, 48), (96, 96))])
    o_first = each_way(lambda h: remote(pk.at[1, h], pk.at[1, 2 + h], h))
    second = [each_way(lambda h: remote(pk.at[m, 1 - h], pk.at[m, 4 + h], h)) for m in range(2)]
    q_fwd = each_way(lambda h: remote(pk.at[0, 2 + h], pk.at[0, 6 + h], h))
    o_fwd = each_way(lambda h: [remote(pk.at[1, 2 + h, pl.ds(o, n)], pk.at[1, 6 + h, pl.ds(o, n)], h)
                                for o, n in ((0, 48), (48, 48), (96, 48), (144, 24), (168, 24))])
    side_own = [each_way(lambda h: remote(side.at[m, 0], side.at[m, 1 + h], h)) for m in range(2)]
    side_fwd = [remote(side.at[m, 1 + m], side.at[m, 3], m) for m in range(2)]
    high_first = [each_way(lambda h: remote(high.at[m, h], high.at[m, 2 + h], h)) for m in range(2)]
    high_second = [each_way(lambda h: remote(high.at[m, 1 - h], high.at[m, 4 + h], h)) for m in range(2)]
    high_fwd = [each_way(lambda h: remote(high.at[m, 2 + h], high.at[m, 6 + h], h)) for m in range(2)]

    h0 = jnp.where(me == 1, 1, 0)
    halves = (h0, 1 - h0)
    wq_rows = ((0, 64), (64, 64), (128, 128), (256, 256))
    wq_loads = [[pltpu.make_async_copy(wq_hbm.at[pl.ds(o, n), pl.ds(pl.multiple_of(128 * halves[s], 128), 128)],
                                       wq_f.at[s, pl.ds(o, n)], ld_wq.at[4 * s + i])
                 for i, (o, n) in enumerate(wq_rows)] for s in range(2)]
    x_loads = [pltpu.make_async_copy(x_hbm.at[pl.ds(256 * b, 256)], x_f.at[pl.ds(256 * b, 256)], ld_x.at[b])
               for b in range(2)]
    wo_load = pltpu.make_async_copy(wo_hbm, wo_f, ld_wo)
    kv_loads = [(pltpu.make_async_copy(k_hbm.at[:, pair_of[c]], k_f.at[c], ld_kv.at[c]),
                 pltpu.make_async_copy(v_hbm.at[:, pair_of[c]], v_f.at[c], ld_kv.at[c])) for c in range(8)]

    def kv_start(c):
        for d in kv_loads[c]:
            d.start()

    def kv_wait(c):
        for d in kv_loads[c]:
            d.wait()

    codes = {}

    def own_words(m, half, o, n):
        return _words(pltpu.bitcast(w_own[m, half, pl.ds(o, n), :], i32))

    def pack(m, half, o, n):
        pk[m, half, pl.ds(3 * o // 8, 3 * n // 8), :] = _pack(own_words(m, half, o, n))

    def write_side(m):
        code, odd = 0, 0
        for half in range(2):
            for g in range(2):
                words = own_words(m, half, 256 * g, 256)
                high[m, half, pl.ds(32 * g, 32), :] = _pack_high(words)
                c, o = _describe(words)
                code, odd = code | (c << (16 * half + 8 * g)), odd | (o << (16 * half + 8 * g))
        row = lax.broadcasted_iota(i32, (8, 128), 0) & 3
        side[m, 0] = odd | ((lax.shift_right_logical(jnp.broadcast_to(code, (8, 128)), 2 * row) & 0x03030303) << 6)
        codes[m, 0] = code[0, 0]

    def read_side(m, o):
        rows = [(lax.shift_right_logical(side[m, o, r:r + 1, :], 6) & 0x03030303) << (2 * r) for r in range(4)]
        codes[m, o] = _tree(jnp.bitwise_or, rows)[0, 0]

    def code_of(m, c, g):
        return lax.shift_right_logical(codes[m, owner[c]], 16 * half_of[c] + 8 * g) & 255

    def odd_of(m, c, g):
        return lax.shift_right_logical(side[m, owner[c]], 16 * half_of[c] + 8 * g) & 63

    def has_full(m, *cs):
        return _tree(jnp.bitwise_or, [code_of(m, c, g) == FULL for c in cs for g in range(2)])

    def weights(m, c, u):
        if c < 2:
            return w_own[m, c, pl.ds(64 * u, 64), :]
        words = _unpack(_words(pk[m, c, pl.ds(24 * u, 24), :]), high[m, c, pl.ds(8 * u, 8), :],
                        code_of(m, c, u // 4), odd_of(m, c, u // 4), u % 4)
        return pltpu.bitcast(jnp.concatenate(words, 0), bf16)

    ka = 3 - lax.rem(me, 3)
    b1 = jnp.where(ka == 2, 3, 2)
    b2 = jnp.where(ka == 1, 3, 1)

    def sees(j, kb):
        qb = 4 * me + j
        return ((qb == kb) | (lax.rem(qb + kb, 3) == 0)).astype(i32)

    def prep(c):
        keep = (lax.broadcasted_iota(i32, (128, 128), 1) < 64) | (ka == 1)
        for b in range(2):
            k_b[c, b] = k_f[c, b].astype(bf16).T
            lo, hi = v_f[c, b, :, 0:128], v_f[c, b, :, 128:256]
            hi = jnp.where(ka == 2, pltpu.roll(hi, 64, 1), hi)
            v_b[c, b, 0] = jnp.where(keep, lo, hi).astype(bf16)
            v_b[c, b, 1] = jnp.where(keep, hi, lo).astype(bf16)

    def project_q(c):
        w = jnp.concatenate([weights(0, c, u) for u in range(8)], 0)
        q = jnp.dot(x_b[...], w, preferred_element_type=f32)
        first = lax.broadcasted_iota(i32, (512, 128), 1) < 64
        q_b[c, 0] = jnp.where(first, q, 0.0).astype(bf16)
        q_b[c, 1] = jnp.where(first, 0.0, q).astype(bf16)

    def scores(c):
        s = {}
        for b in range(2):
            k0 = k_b[c, b, 0:64, :]
            ks = [k_b[c, b, pl.ds(pl.multiple_of(64 * kb, 64), 64), :] for kb in (ka, b1, b2)]
            keys = (jnp.concatenate([k0, ks[0]], 0), jnp.concatenate([k0, ks[1], ks[2]], 0))
            for h in range(2):
                q = (jnp.concatenate([q_b[c, h, pl.ds(256 * b, 64), :], q_b[c, h, pl.ds(256 * b + 192, 64), :]], 0),
                     q_b[c, h, pl.ds(256 * b + 64, 128), :])
                for t in range(2):
                    s[b, h, t] = lax.dot_general(keys[t], q[t], (((1,), (1,)), ((), ())),
                                                 preferred_element_type=f32)
        return s

    def attend(c, s):
        first = lax.broadcasted_iota(i32, (64, 128), 1) < 64
        seen = [jnp.where(first, sees(1, kb), sees(2, kb)) > 0 for kb in (b1, b2)]
        p = {}
        for (b, h, t), x in s.items():
            if t == 1:
                x = jnp.concatenate(
                    [x[:64], jnp.where(seen[0], x[64:128], -1e9), jnp.where(seen[1], x[128:], -1e9)], 0)
            e = jnp.exp2(x - jnp.max(x, axis=0, keepdims=True))
            p[b, h, t] = e, 1.0 / jnp.sum(e, axis=0, keepdims=True)
        for (b, h, t), (e, inv) in p.items():
            v = v_b[c, b, 0, 64 * h:64 * h + 64, :]
            if t == 1:
                v = jnp.concatenate([v, v_b[c, b, 1, 64 * h:64 * h + 64, :]], 1)
                e = jnp.concatenate([e[:64], jnp.zeros((64, 128), f32), e[64:]], 0)
            o = jnp.dot(v, e.astype(bf16), preferred_element_type=f32) * inv
            tile, place = (c, h) if c < 6 else (6 + h, c - 6)
            o_t[tile, b, t, pl.ds(64 * place, 64), :] = o.astype(bf16)

    def put_ctx(c):
        for b in range(2):
            a = o_t[c, b, 0].T
            ctx[c, pl.ds(256 * b, 64), :] = a[:64]
            ctx[c, pl.ds(256 * b + 64, 128), :] = o_t[c, b, 1].T
            ctx[c, pl.ds(256 * b + 192, 64), :] = a[64:]

    def project_out(cs, w, parts):
        rows = 512 // parts
        return jnp.concatenate(
            [jnp.dot(jnp.concatenate([ctx[c, pl.ds(r * rows, rows), :] for c in cs], 1), w,
                     preferred_element_type=f32) for r in range(parts)], 0)

    def wo_tiles(cs, n):
        return jnp.concatenate([weights(1, c, u) for c in cs for u in (2 * n, 2 * n + 1)], 0)

    wq_order = ((0, 0), (0, 1), (1, 0), (1, 1), (0, 2), (1, 2), (0, 3), (1, 3))
    for s, i in wq_order[:2]:
        wq_loads[s][i].start()
    barrier = pltpu.get_barrier_semaphore()

    @pl.when(me != 2)
    def _():
        for other in (left, right):
            pl.semaphore_signal(barrier, inc=1, device_id=(other,), device_id_type=MESH)

    for s, i in wq_order[2:]:
        wq_loads[s][i].start()

    @pl.when(me != 0)
    def _():
        pl.semaphore_wait(barrier, 2 - (me & 1))

    @pl.when(me == 2)
    def _():
        for other in (left, right):
            pl.semaphore_signal(ready, inc=1, device_id=(other,), device_id_type=MESH)

    may_send = (me >= 2, (me == 1) | (me == 2))
    for s, i in wq_order:
        o, n = wq_rows[i]
        wq_loads[s][i].wait()
        w_own[0, halves[s], pl.ds(o, n), :] = wq_f[s, pl.ds(o, n), :].astype(bf16)
        pack(0, halves[s], o, n)
        for h in range(2):
            pl.when(may_send[h] & (halves[s] == h))(q_first[h][i].start)
        if (s, i) == wq_order[1]:
            for d in x_loads:
                d.start()
    kv_start(0)

    @pl.when((me & 1) == 1)
    def _():
        pl.semaphore_wait(ready, 1)
        for h in range(2):
            @pl.when(jnp.logical_not(may_send[h]))
            def _():
                for d in q_first[h]:
                    d.start()

    write_side(0)

    @pl.when(me == 0)
    def _():
        pl.semaphore_wait(barrier, 2)
        for pieces in zip(*q_first):
            for d in pieces:
                d.start()

    for h in range(2):
        side_own[0][h].start()

    @pl.when(has_full(0, 0, 1))
    def _():
        for h in range(2):
            pl.when(has_full(0, h))(high_first[0][h].start)
            pl.when(has_full(0, 1 - h))(high_second[0][h].start)

    for h in range(2):
        second[0][h].start()

    for b in range(2):
        x_loads[b].wait()
        x_b[pl.ds(256 * b, 256), :] = (x_f[pl.ds(256 * b, 256), :] * SCALE).astype(bf16)
        if b == 0:
            wo_load.start()
    project_q(0)

    kv_wait(0)
    kv_start(1)
    prep(0)
    project_q(1)

    wo_load.wait()
    kv_start(2)
    for h in range(2):
        for n in range(4):
            w_own[1, h, pl.ds(128 * n, 128), :] = wo_f[128 * h:128 * h + 128, 128 * n:128 * n + 128].astype(bf16)
        pack(1, h, 0, 512)
    write_side(1)
    for h in range(2):
        side_own[1][h].start()
        o_first[h].start()

    @pl.when(has_full(1, 0, 1))
    def _():
        for h in range(2):
            pl.when(has_full(1, h))(high_first[1][h].start)
            pl.when(has_full(1, 1 - h))(high_second[1][h].start)

    kv_start(3)
    attend(0, scores(0))

    kv_wait(1)
    kv_start(4)
    for h in range(2):
        side_own[0][h].wait_recv()
    for h in range(2):
        read_side(0, 1 + h)
    side_fwd[0].start()
    for h in range(2):
        for d in q_first[h]:
            d.wait_recv()

    @pl.when(has_full(0, 2, 3))
    def _():
        for h in range(2):
            pl.when(has_full(0, 2 + h))(high_first[0][h].wait_recv)
            pl.when(has_full(0, 2 + h))(high_fwd[0][h].start)

    for h in range(2):
        q_fwd[h].start()
        second[1][h].start()
    put_ctx(0)
    prep(1)
    project_q(2)

    kv_wait(2)
    kv_start(5)
    prep(2)
    s = scores(1)
    project_q(3)
    attend(1, s)

    kv_wait(3)
    kv_start(6)
    put_ctx(1)
    prep(3)
    attend(2, scores(2))

    kv_wait(4)
    kv_start(7)
    for h in range(2):
        second[0][h].wait_recv()

    @pl.when(has_full(0, 4, 5))
    def _():
        for h in range(2):
            pl.when(has_full(0, 4 + h))(high_second[0][h].wait_recv)

    for c in (3, 4):
        if c == 4:
            kv_wait(5)
        put_ctx(c - 1)
        prep(c + 1)
        s = scores(c)
        project_q(c + 1)
        attend(c, s)

    kv_wait(6)
    kv_wait(7)
    for h in range(2):
        side_own[1][h].wait_recv()
    side_fwd[0].wait_recv()
    for h in range(2):
        read_side(1, 1 + h)
    read_side(0, 3)
    side_fwd[1].start()
    for h in range(2):
        o_first[h].wait_recv()

    @pl.when(has_full(1, 2, 3, 4, 5))
    def _():
        for h in range(2):
            pl.when(has_full(1, 2 + h))(high_first[1][h].wait_recv)
            pl.when(has_full(1, 2 + h))(high_fwd[1][h].start)
            pl.when(has_full(1, 4 + h))(high_second[1][h].wait_recv)

    for pieces in zip(*o_fwd):
        for d in pieces:
            d.start()
    put_ctx(4)
    prep(6)
    prep(7)
    s = scores(5)
    for n in range(4):
        acc[:, 128 * n:128 * n + 128] = project_out((0, 1, 2, 3), wo_tiles((0, 1, 2, 3), n), 1)
        if n == 1:
            attend(5, s)

    for h in range(2):
        q_fwd[h].wait_recv()

    @pl.when(has_full(0, 6, 7))
    def _():
        for h in range(2):
            pl.when(has_full(0, 6 + h))(high_fwd[0][h].wait_recv)

    put_ctx(5)
    project_q(6)
    s = scores(6)
    project_q(7)
    attend(6, s)
    attend(7, scores(7))

    for h in range(2):
        second[1][h].wait_recv()
    side_fwd[1].wait_recv()
    read_side(1, 3)
    put_ctx(6)
    put_ctx(7)
    for n in range(4):
        acc[:, 128 * n:128 * n + 128] += project_out((4, 5), wo_tiles((4, 5), n), 2)

    @pl.when(has_full(1, 6, 7))
    def _():
        for h in range(2):
            pl.when(has_full(1, 6 + h))(high_fwd[1][h].wait_recv)

    for i, (n, hs) in enumerate(((0, (0, 1)), (1, (0, 1)), (2, (0, 1)), (3, (0,)), (3, (1,)))):
        if i == 2:
            for h in range(2):
                for d in (*q_first[h], o_first[h], second[0][h], second[1][h], q_fwd[h], *o_fwd[h],
                          side_own[0][h], side_own[1][h], side_fwd[h]):
                    d.wait_send()

            @pl.when(has_full(0, 0, 1, 2, 3) | has_full(1, 0, 1, 2, 3))
            def _():
                for h in range(2):
                    for m in range(2):
                        pl.when(has_full(m, h))(high_first[m][h].wait_send)
                        pl.when(has_full(m, 1 - h))(high_second[m][h].wait_send)
                        pl.when(has_full(m, 2 + h))(high_fwd[m][h].wait_send)

        for h in range(2):
            o_fwd[h][i].wait_recv()
        cols = pl.ds(128 * n, 128)
        w = jnp.concatenate([weights(1, c, 2 * n + h) for h in hs for c in (6, 7)], 0)
        total = acc[:, cols] + project_out([6 + h for h in hs], w, 4 // len(hs))
        if hs[-1] == 1:
            out_ref[:, cols] = total.astype(out_ref.dtype)
        else:
            acc[:, cols] = total


def pallas_dist_sparse_attn_blocksparse_qseq_b2_sq256_skv256_hq4_dh64_kernel(
    x: jax.Array,
    Wq: jax.Array,
    K_ext: jax.Array,
    V_ext: jax.Array,
    Wo: jax.Array,
):
    kt = jnp.transpose(K_ext, (0, 2, 3, 1)).reshape(2, 8, 128, 256)
    vt = jnp.transpose(V_ext, (0, 2, 3, 1)).reshape(2, 8, 128, 256)
    vmem, dma = pltpu.VMEM, pltpu.SemaphoreType.DMA
    out = pl.pallas_call(
        _body,
        out_shape=jax.ShapeDtypeStruct((512, 512), bf16),
        in_specs=[pl.BlockSpec(memory_space=pltpu.HBM)] * 5,
        out_specs=pl.BlockSpec(memory_space=pltpu.VMEM),
        scratch_shapes=[
            vmem((512, 512), f32), vmem((512, 512), bf16),
            vmem((2, 512, 128), f32), vmem((256, 512), f32),
            vmem((8, 2, 128, 256), f32), vmem((8, 2, 128, 256), f32),
            vmem((8, 2, 256, 128), bf16), vmem((8, 2, 2, 128, 128), bf16),
            vmem((2, 2, 512, 128), bf16), vmem((2, 8, 192, 128), i32),
            vmem((2, 8, 64, 128), i32), vmem((2, 4, 8, 128), i32),
            vmem((8, 2, 512, 128), bf16), vmem((8, 2, 2, 128, 128), bf16),
            vmem((8, 512, 128), bf16), vmem((512, 512), f32),
            dma((8,)), dma((2,)), dma, dma((8,)),
            dma((NUM_REMOTE,)), dma((NUM_REMOTE,)), pltpu.SemaphoreType.REGULAR,
        ],
        compiler_params=pltpu.CompilerParams(
            collective_id=0, vmem_limit_bytes=64 * 2**20, disable_semaphore_checks=True),
    )(x.reshape(512, 512), Wq, kt, vt, Wo)
    return out.reshape(2, 256, 512)
```
